```python
import numpy as np

kernel_name = "dist_argmax_global_i_m4096_n1024"

def setup_inputs():
    return {"x": np.random.randn(16384, 1024).astype(np.float32)}

def reference(x: np.ndarray) -> np.ndarray:
    idx = np.argmax(x, axis=0).astype(np.float32)
    val = np.max(x, axis=0)
    return np.stack([val, idx], axis=0)
```

```python
import jax
import jax.numpy as jnp
from jax import lax
from jax.experimental import pallas as pl
from jax.experimental.pallas import tpu as pltpu
from jax.experimental.pallas.tpu import CompilerParams

N_DEV = 4
M, N = 4096, 1024
G = N // 128

K_PUSH = 208
M_OWN = M - 2 * K_PUSH
CHUNKS = (2104, 1024, 384, 128, 32, 8)
PUSH_AFTER = 1
UNROLL = 8

FBIAS = float(1 << 23)
BIG = float(1 << 24)

assert sum(CHUNKS) == M_OWN
assert N_DEV * M <= 1 << 15


def _tree(f, xs):
    while len(xs) > 1:
        xs = [f(*xs[i : i + 2]) if i + 1 < len(xs) else xs[i] for i in range(0, len(xs), 2)]
    return xs[0]


def _scan(ref, lo, rows, carry):
    top = (lo + rows) // 8 - 1
    steps = rows // 8

    def step(t, c):
        best, base = c
        r = top - t
        v = ref[pl.ds(pl.multiple_of(r * 8, 8), 8), :]
        take = (v >= best) | (v != v)
        return jnp.where(take, v, best), jnp.where(take, (r * 8).astype(jnp.float32), base)

    return lax.fori_loop(0, steps, step, carry, unroll=min(UNROLL, steps))


def _scan_init():
    return jnp.full((8, N), -jnp.inf, jnp.float32), jnp.zeros((8, N), jnp.float32)


def _pack_groups(x):
    sub = lax.broadcasted_iota(jnp.int32, (8, 128), 0)
    vals = [jnp.broadcast_to(x[:, g * 128 : (g + 1) * 128], (8, 128)) for g in range(G)]
    for bit in (1, 2, 4):
        vals = [
            jnp.where((sub & bit) == 0, vals[i], vals[i + 1]) for i in range(0, len(vals), 2)
        ]
    return vals[0]


def _reduce_sublanes(best, base, row0):
    mx = jnp.max(best, axis=0, keepdims=True)
    sub = lax.broadcasted_iota(jnp.int32, (8, N), 0)
    idx = base + ((sub + row0).astype(jnp.float32) + FBIAS)
    hit = (best == mx) | (best != best)
    ix = jnp.min(jnp.where(hit, idx, BIG), axis=0, keepdims=True)
    return _pack_groups(mx), _pack_groups(ix)


def _merge(parts):
    gm = _tree(jnp.maximum, [v for v, _ in parts])
    gi = _tree(jnp.minimum, [jnp.where((v == gm) | (v != v), i, BIG) for v, i in parts])
    return gm, gi


def _body(x_hbm, out_ref, buf, fbuf, msg, in_sems, push_send, push_recv, send_sems, recv_sems):
    n_chunks = len(CHUNKS)
    los = [M_OWN - sum(CHUNKS[: j + 1]) for j in range(n_chunks)]

    def local_copy(j):
        rows = pl.ds(los[j], CHUNKS[j])
        return pltpu.make_async_copy(x_hbm.at[rows], buf.at[rows], in_sems.at[j])

    for j in range(n_chunks):
        local_copy(j).start()

    my = lax.axis_index("i")

    def peer(d):
        return ((my + d) & (N_DEV - 1),)

    barrier = pltpu.get_barrier_semaphore()
    for d in range(1, N_DEV):
        pl.semaphore_signal(barrier, inc=1, device_id=peer(d), device_id_type=pl.DeviceIdType.MESH)
    pl.semaphore_wait(barrier, N_DEV - 1)

    push_to = (1, N_DEV - 1)

    def push(q):
        return pltpu.make_async_remote_copy(
            x_hbm.at[pl.ds(M_OWN + q * K_PUSH, K_PUSH)],
            fbuf.at[q],
            push_send.at[q],
            push_recv.at[q],
            device_id=peer(push_to[q]),
            device_id_type=pl.DeviceIdType.MESH,
        )

    for q in range(2):
        push(q).start()

    carry = _scan_init()
    foreign = None
    for j in range(n_chunks):
        local_copy(j).wait()
        carry = _scan(buf, los[j], CHUNKS[j], carry)
        if j == PUSH_AFTER:
            parts = []
            for q in range(2):
                push(q).wait_recv()
                src = (my - push_to[q]) & (N_DEV - 1)
                fb = _scan(fbuf.at[q], 0, K_PUSH, _scan_init())
                parts.append(_reduce_sublanes(*fb, src * M + (M_OWN + q * K_PUSH)))
            foreign = _merge(parts)
            for q in range(2):
                push(q).wait_send()

    val, idx = _merge([_reduce_sublanes(*carry, my * M), foreign])

    idx16 = lax.bitcast_convert_type(idx, jnp.int32).astype(jnp.int16)
    msg[my, 0:8, :] = val
    msg[my, 8:12, :] = lax.bitcast_convert_type(pltpu.bitcast(idx16, jnp.int32), jnp.float32)

    sends = []
    for j, d in enumerate((2, 1, 3)):
        rdma = pltpu.make_async_remote_copy(
            msg.at[my],
            msg.at[my],
            send_sems.at[j],
            recv_sems.at[my],
            device_id=peer(d),
            device_id_type=pl.DeviceIdType.MESH,
        )
        rdma.start()
        sends.append(rdma)
    for rdma in sends:
        rdma.wait_send()
    for d in (1, 3, 2):
        src = (my + d) & (N_DEV - 1)
        pltpu.make_async_remote_copy(
            msg.at[src],
            msg.at[src],
            send_sems.at[0],
            recv_sems.at[src],
            device_id=(src,),
            device_id_type=pl.DeviceIdType.MESH,
        ).wait_recv()

    parts = []
    for s in range(N_DEV):
        i16 = pltpu.bitcast(lax.bitcast_convert_type(msg[s, 8:12, :], jnp.int32), jnp.int16)
        parts.append((msg[s, 0:8, :], i16.astype(jnp.int32).astype(jnp.float32)))
    val, idx = _merge(parts)
    out_ref[0:1, :] = val.reshape(1, N)
    out_ref[1:2, :] = idx.reshape(1, N)


def pallas_dist_argmax_global_i_m4096_n1024_kernel(x: jax.Array):
    return pl.pallas_call(
        _body,
        out_shape=jax.ShapeDtypeStruct((2, N), jnp.float32),
        in_specs=[pl.BlockSpec(memory_space=pl.ANY)],
        out_specs=pl.BlockSpec(memory_space=pltpu.VMEM),
        scratch_shapes=[
            pltpu.VMEM((M_OWN, N), jnp.float32),
            pltpu.VMEM((2, K_PUSH, N), jnp.float32),
            pltpu.VMEM((N_DEV, 12, 128), jnp.float32),
            pltpu.SemaphoreType.DMA((len(CHUNKS),)),
            pltpu.SemaphoreType.DMA((2,)),
            pltpu.SemaphoreType.DMA((2,)),
            pltpu.SemaphoreType.DMA((N_DEV - 1,)),
            pltpu.SemaphoreType.DMA((N_DEV,)),
        ],
        compiler_params=CompilerParams(
            collective_id=0,
            vmem_limit_bytes=48 * 1024 * 1024,
            disable_semaphore_checks=True,
        ),
    )(x)
```

```python
import jax
import jax.numpy as jnp
from jax import lax
from jax.experimental import pallas as pl
from jax.experimental.pallas import tpu as pltpu
from jax.experimental.pallas.tpu import CompilerParams

N_DEV = 4
M, N = 4096, 1024
G = N // 128

K_PUSH = 200
M_OWN = M - 2 * K_PUSH
PUSH_TO = (1, N_DEV - 1)
CHUNKS = (2032, 1024, 384, 128)
PUSH_AFTER = 1
R_LAST = 128
BLOCKS = (4, 2, 1, 1)
UNROLL = 8
BIG = float(1 << 24)

assert sum(CHUNKS) + R_LAST == M_OWN and sum(BLOCKS) == G
assert all(c % 8 == 0 for c in (*CHUNKS, R_LAST, K_PUSH))


def _tree(f, xs):
    while len(xs) > 1:
        xs = [f(*xs[i : i + 2]) if i + 1 < len(xs) else xs[i] for i in range(0, len(xs), 2)]
    return xs[0]


def _lanes(g, n=1):
    return slice(g * 128, (g + n) * 128)


def _keep_first(later, earlier):
    v = earlier[0]
    take = (v >= later[0]) | (v != v)
    return jnp.where(take, v, later[0]), jnp.where(take, earlier[1], later[1])


def _scan(ref, lo, rows, carry):
    top = (lo + rows) // 8 - 1
    steps = rows // 8

    def step(t, c):
        r = top - t
        rs = pl.ds(pl.multiple_of(r * 8, 8), 8)
        base = (r * 8).astype(jnp.float32)
        return tuple(_keep_first(c[g], (ref[rs, _lanes(g)], base)) for g in range(G))

    return lax.fori_loop(0, steps, step, carry, unroll=min(UNROLL, steps))


def _scan_init():
    init = jnp.full((8, 128), -jnp.inf, jnp.float32), jnp.zeros((8, 128), jnp.float32)
    return (init,) * G


def _reduce_sublanes(best, base, row0, other=None):
    mx = jnp.max(best, axis=0, keepdims=True)
    if other is not None:
        mx = jnp.maximum(mx, other[0])
    sub = lax.broadcasted_iota(jnp.int32, (8, 128), 0)
    idx = base + (sub + row0).astype(jnp.float32)
    ix = jnp.min(_index_if_hit((best, idx), mx), axis=0, keepdims=True)
    if other is not None:
        ix = jnp.minimum(ix, _index_if_hit(other, mx))
    return mx, ix


def _index_if_hit(cand, mx):
    v, i = cand
    return jnp.where((v == mx) | (v != v), i, BIG)


def _merge(cands):
    mx = _tree(jnp.maximum, [v for v, _ in cands])
    return mx, _tree(jnp.minimum, [_index_if_hit(c, mx) for c in cands])


def _body(
    x_hbm, out_ref, buf, fbuf, msg,
    chunk_sems, block_sems, push_send, push_recv, far_send, far_recv, near_send, near_recv,
):
    n_chunks, n_blocks = len(CHUNKS), len(BLOCKS)
    los = [M_OWN - sum(CHUNKS[: j + 1]) for j in range(n_chunks)]
    g0s = [sum(BLOCKS[:j]) for j in range(n_blocks)]

    def chunk_copy(j):
        rows = pl.ds(los[j], CHUNKS[j])
        return pltpu.make_async_copy(x_hbm.at[rows], buf.at[rows], chunk_sems.at[j])

    def block_copy(j):
        at = (pl.ds(0, R_LAST), pl.ds(g0s[j] * 128, BLOCKS[j] * 128))
        return pltpu.make_async_copy(x_hbm.at[at], buf.at[at], block_sems.at[j])

    for j in range(n_chunks):
        chunk_copy(j).start()
    for j in range(n_blocks):
        block_copy(j).start()

    my = lax.axis_index("i")

    def chip(d):
        return (my + d) & (N_DEV - 1)

    def remote(src, dst, send_sem, recv_sem, d):
        return pltpu.make_async_remote_copy(
            src, dst, send_sem, recv_sem,
            device_id=(chip(d),), device_id_type=pl.DeviceIdType.MESH,
        )

    barrier = pltpu.get_barrier_semaphore()
    for d in range(1, N_DEV):
        pl.semaphore_signal(
            barrier, inc=1, device_id=(chip(d),), device_id_type=pl.DeviceIdType.MESH
        )
    pl.semaphore_wait(barrier, N_DEV - 1)

    def push(q):
        rows = pl.ds(M_OWN + q * K_PUSH, K_PUSH)
        return remote(x_hbm.at[rows], fbuf.at[q], push_send.at[q], push_recv.at[q], PUSH_TO[q])

    for q in range(2):
        push(q).start()

    carry = _scan_init()
    foreign = None
    for j in range(n_chunks):
        chunk_copy(j).wait()
        carry = _scan(buf, los[j], CHUNKS[j], carry)
        if j == PUSH_AFTER:
            parts = []
            for q in range(2):
                push(q).wait_recv()
                row0 = chip(-PUSH_TO[q]) * M + (M_OWN + q * K_PUSH)
                folded = _scan(fbuf.at[q], 0, K_PUSH, _scan_init())
                parts.append([_reduce_sublanes(*c, row0) for c in folded])
            foreign = [_merge(p) for p in zip(*parts)]
            for q in range(2):
                push(q).wait_send()

    def far(s, j):
        part = msg.at[s, pl.ds(g0s[j], BLOCKS[j])]
        return remote(part, part, far_send.at[j], far_recv.at[j], 2)

    def near(s, q):
        return remote(msg.at[s], msg.at[s], near_send.at[q], near_recv.at[q], PUSH_TO[q])

    for j in range(n_blocks):
        block_copy(j).wait()
        for g in range(g0s[j], g0s[j] + BLOCKS[j]):
            cands = [carry[g]] + [
                (buf[r : r + 8, _lanes(g)], float(r)) for r in range(R_LAST - 8, -1, -8)
            ]
            if BLOCKS[j] > 2:
                best = cands[0]
                for c in cands[1:]:
                    best = _keep_first(best, c)
            else:
                best = _tree(_keep_first, cands)
            mx, ix = _reduce_sublanes(*best, my * M, foreign[g])
            msg[my, g, 0:1, :] = mx
            msg[my, g, 1:2, :] = ix
        far(my, j).start()
    for q in range(2):
        near(my, q).start()

    for q in range(2):
        near(chip(-PUSH_TO[q]), q).wait_recv()
    for j in range(n_blocks):
        far(my, j).wait_send()
    for q in range(2):
        near(my, q).wait_send()
    for j in range(n_blocks):
        far(chip(2), j).wait_recv()
        gs = slice(g0s[j], g0s[j] + BLOCKS[j])
        mx, ix = _merge([(msg[s, gs, 0, :], msg[s, gs, 1, :]) for s in range(N_DEV)])
        out_ref[0:1, _lanes(g0s[j], BLOCKS[j])] = mx.reshape(1, BLOCKS[j] * 128)
        out_ref[1:2, _lanes(g0s[j], BLOCKS[j])] = ix.reshape(1, BLOCKS[j] * 128)


def pallas_dist_argmax_global_i_m4096_n1024_kernel(x: jax.Array):
    dma = pltpu.SemaphoreType.DMA
    return pl.pallas_call(
        _body,
        out_shape=jax.ShapeDtypeStruct((2, N), jnp.float32),
        in_specs=[pl.BlockSpec(memory_space=pl.ANY)],
        out_specs=pl.BlockSpec(memory_space=pltpu.VMEM),
        scratch_shapes=[
            pltpu.VMEM((M_OWN, N), jnp.float32),
            pltpu.VMEM((2, K_PUSH, N), jnp.float32),
            pltpu.VMEM((N_DEV, G, 2, 128), jnp.float32),
            dma((len(CHUNKS),)),
            dma((len(BLOCKS),)),
            dma((2,)),
            dma((2,)),
            dma((len(BLOCKS),)),
            dma((len(BLOCKS),)),
            dma((2,)),
            dma((2,)),
        ],
        compiler_params=CompilerParams(
            collective_id=0,
            vmem_limit_bytes=48 * 1024 * 1024,
            disable_semaphore_checks=True,
        ),
    )(x)
```

```python
import jax
import jax.numpy as jnp
from jax import lax
from jax.experimental import pallas as pl
from jax.experimental.pallas import tpu as pltpu
from jax.experimental.pallas.tpu import CompilerParams

N_DEV = 4
M, N = 4096, 1024
G = N // 128

K_PUSH = 200
M_OWN = M - 2 * K_PUSH
PUSH_TO = (1, N_DEV - 1)
CHUNKS = (2032, 1024, 384, 128)
PUSH_AFTER = 1
R_LAST = 128
BLOCKS = (
    (0, 4, ((0, R_LAST),)),
    (4, 2, ((0, R_LAST),)),
    (6, 1, ((0, R_LAST),)),
    (7, 1, ((32, R_LAST), (0, 32))),
)
PIECES = tuple((g0, ng, lo, hi) for g0, ng, ranges in BLOCKS for lo, hi in ranges)
UNROLL = 8
BIG = float(1 << 24)

assert sum(CHUNKS) + R_LAST == M_OWN and sum(ng for _, ng, _ in BLOCKS) == G
assert all(c % 8 == 0 for c in (*CHUNKS, K_PUSH, *(r for p in PIECES for r in p[2:])))


def _tree(f, xs):
    while len(xs) > 1:
        xs = [f(*xs[i : i + 2]) if i + 1 < len(xs) else xs[i] for i in range(0, len(xs), 2)]
    return xs[0]


def _lanes(g, n=1):
    return slice(g * 128, (g + n) * 128)


def _keep_first(later, earlier):
    v = earlier[0]
    take = (v >= later[0]) | (v != v)
    return jnp.where(take, v, later[0]), jnp.where(take, earlier[1], later[1])


def _scan(ref, lo, rows, carry):
    top = (lo + rows) // 8 - 1
    steps = rows // 8

    def step(t, c):
        r = top - t
        rs = pl.ds(pl.multiple_of(r * 8, 8), 8)
        base = (r * 8).astype(jnp.float32)
        return tuple(_keep_first(c[g], (ref[rs, _lanes(g)], base)) for g in range(G))

    return lax.fori_loop(0, steps, step, carry, unroll=min(UNROLL, steps))


def _scan_init():
    init = jnp.full((8, 128), -jnp.inf, jnp.float32), jnp.zeros((8, 128), jnp.float32)
    return (init,) * G


def _reduce_sublanes(best, base, row0, other=None):
    mx = jnp.max(best, axis=0, keepdims=True)
    if other is not None:
        mx = jnp.maximum(mx, other[0])
    sub = lax.broadcasted_iota(jnp.int32, (8, 128), 0)
    idx = base + (sub + row0).astype(jnp.float32)
    ix = jnp.min(_index_if_hit((best, idx), mx), axis=0, keepdims=True)
    if other is not None:
        ix = jnp.minimum(ix, _index_if_hit(other, mx))
    return mx, ix


def _index_if_hit(cand, mx):
    v, i = cand
    return jnp.where((v == mx) | (v != v), i, BIG)


def _merge(cands):
    mx = _tree(jnp.maximum, [v for v, _ in cands])
    return mx, _tree(jnp.minimum, [_index_if_hit(c, mx) for c in cands])


def _body(
    x_hbm, out_ref, buf, fbuf, msg,
    chunk_sems, piece_sems, push_send, push_recv, far_send, far_recv, near_send, near_recv,
):
    n_chunks, n_blocks = len(CHUNKS), len(BLOCKS)
    los = [M_OWN - sum(CHUNKS[: j + 1]) for j in range(n_chunks)]

    def chunk_copy(j):
        rows = pl.ds(los[j], CHUNKS[j])
        return pltpu.make_async_copy(x_hbm.at[rows], buf.at[rows], chunk_sems.at[j])

    def piece_copy(piece):
        g0, ng, lo, hi = piece
        at = (pl.ds(lo, hi - lo), pl.ds(g0 * 128, ng * 128))
        sem = piece_sems.at[PIECES.index(piece)]
        return pltpu.make_async_copy(x_hbm.at[at], buf.at[at], sem)

    for j in range(n_chunks):
        chunk_copy(j).start()
    for piece in PIECES:
        piece_copy(piece).start()

    my = lax.axis_index("i")

    def chip(d):
        return (my + d) & (N_DEV - 1)

    def remote(src, dst, send_sem, recv_sem, d):
        return pltpu.make_async_remote_copy(
            src, dst, send_sem, recv_sem,
            device_id=(chip(d),), device_id_type=pl.DeviceIdType.MESH,
        )

    barrier = pltpu.get_barrier_semaphore()
    for d in range(1, N_DEV):
        pl.semaphore_signal(
            barrier, inc=1, device_id=(chip(d),), device_id_type=pl.DeviceIdType.MESH
        )
    pl.semaphore_wait(barrier, N_DEV - 1)

    def push(q):
        rows = pl.ds(M_OWN + q * K_PUSH, K_PUSH)
        return remote(x_hbm.at[rows], fbuf.at[q], push_send.at[q], push_recv.at[q], PUSH_TO[q])

    for q in range(2):
        push(q).start()

    carry = _scan_init()
    foreign = None
    for j in range(n_chunks):
        chunk_copy(j).wait()
        carry = _scan(buf, los[j], CHUNKS[j], carry)
        if j == PUSH_AFTER:
            parts = []
            for q in range(2):
                push(q).wait_recv()
                row0 = chip(-PUSH_TO[q]) * M + (M_OWN + q * K_PUSH)
                folded = _scan(fbuf.at[q], 0, K_PUSH, _scan_init())
                parts.append([_reduce_sublanes(*c, row0) for c in folded])
            foreign = [_merge(p) for p in zip(*parts)]
            for q in range(2):
                push(q).wait_send()

    def far(s, j):
        part = msg.at[s, pl.ds(*BLOCKS[j][:2])]
        return remote(part, part, far_send.at[j], far_recv.at[j], 2)

    def near(s, q):
        return remote(msg.at[s], msg.at[s], near_send.at[q], near_recv.at[q], PUSH_TO[q])

    carry = list(carry)
    for j, (g0, ng, ranges) in enumerate(BLOCKS):
        for lo, hi in ranges:
            piece_copy((g0, ng, lo, hi)).wait()
            for g in range(g0, g0 + ng):
                cands = [carry[g]] + [
                    (buf[r : r + 8, _lanes(g)], float(r)) for r in range(hi - 8, lo - 1, -8)
                ]
                if ng > 2:
                    for c in cands[1:]:
                        carry[g] = _keep_first(carry[g], c)
                else:
                    carry[g] = _tree(_keep_first, cands)
        for g in range(g0, g0 + ng):
            mx, ix = _reduce_sublanes(*carry[g], my * M, foreign[g])
            msg[my, g, 0:1, :] = mx
            msg[my, g, 1:2, :] = ix
        far(my, j).start()
    for q in range(2):
        near(my, q).start()

    for q in range(2):
        near(chip(-PUSH_TO[q]), q).wait_recv()
    for j in range(n_blocks):
        far(my, j).wait_send()
    for q in range(2):
        near(my, q).wait_send()
    for j, (g0, ng, _) in enumerate(BLOCKS):
        far(chip(2), j).wait_recv()
        gs = slice(g0, g0 + ng)
        mx, ix = _merge([(msg[s, gs, 0, :], msg[s, gs, 1, :]) for s in range(N_DEV)])
        out_ref[0:1, _lanes(g0, ng)] = mx.reshape(1, ng * 128)
        out_ref[1:2, _lanes(g0, ng)] = ix.reshape(1, ng * 128)


def pallas_dist_argmax_global_i_m4096_n1024_kernel(x: jax.Array):
    dma = pltpu.SemaphoreType.DMA
    return pl.pallas_call(
        _body,
        out_shape=jax.ShapeDtypeStruct((2, N), jnp.float32),
        in_specs=[pl.BlockSpec(memory_space=pl.ANY)],
        out_specs=pl.BlockSpec(memory_space=pltpu.VMEM),
        scratch_shapes=[
            pltpu.VMEM((M_OWN, N), jnp.float32),
            pltpu.VMEM((2, K_PUSH, N), jnp.float32),
            pltpu.VMEM((N_DEV, G, 2, 128), jnp.float32),
            dma((len(CHUNKS),)),
            dma((len(PIECES),)),
            dma((2,)),
            dma((2,)),
            dma((len(BLOCKS),)),
            dma((len(BLOCKS),)),
            dma((2,)),
            dma((2,)),
        ],
        compiler_params=CompilerParams(
            collective_id=0,
            vmem_limit_bytes=24 * 1024 * 1024,
        ),
    )(x)
```
